```python
import numpy as np

kernel_name = "dist_moe_cap_ep_outshard_n2048_d512_e8_h1024"

def setup_inputs():
    x = np.random.randn(2048, 512).astype(np.float32)
    router_W = np.random.randn(512, 32).astype(np.float32) * 0.1
    scores64 = x.astype(np.float64) @ router_W.astype(np.float64)
    route_idx = np.argsort(-scores64, axis=-1)[:, :1].astype(np.int32)
    expert_W = np.random.randn(32, 512, 1024).astype(np.float32) * 0.02
    return {"x": x, "router_W": router_W, "route_idx": route_idx, "expert_W": expert_W}

def reference(x, router_W, route_idx, expert_W):
    counts = np.zeros(32, dtype=np.int64)
    out = np.zeros((2048, 1024), dtype=np.float32)
    for i in range(2048):
        e = int(route_idx[i, 0])
        if counts[e] < 51:
            out[i] = x[i] @ expert_W[e]
            counts[e] += 1
    return out
```

```python
import jax
import jax.numpy as jnp
from jax import lax
from jax.experimental import pallas as pl
from jax.experimental.pallas import tpu as pltpu

N_DEV = 4
N_TOK = 2048
D = 512
H = 1024
E_LOC = 8
CAP = 51
SLOTS = 64
ROWS = N_TOK // N_DEV
MESH = pl.DeviceIdType.MESH

UNITS = tuple((e, 0, H) for e in range(E_LOC - 1)) + (
    (E_LOC - 1, 0, H // 2), (E_LOC - 1, H // 2, H // 2))
PLACE_AFTER = {3: (0, 1), 4: (2,), 5: (3,), 6: (4,), 8: (5, 6, 7, 8)}

f32, bf16, i32, u32 = jnp.float32, jnp.bfloat16, jnp.int32, jnp.uint32


def _words(width):
    return width // 256


_STAGE_AT = [0]
for _, _, _w in UNITS:
    _STAGE_AT.append(_STAGE_AT[-1] + N_DEV * SLOTS * _words(_w))


def _body(route_hbm, x_hbm, w_hbm, out_ref,
          route_ref, wv, xg, stage, tab_v, tab_s,
          wsem, gsem, tsem, ssem, rsem, done_sem):
    me = lax.axis_index("i")

    route_copy = pltpu.make_async_copy(route_hbm, route_ref, tsem)
    route_copy.start()

    def w_copy(u):
        e, c0, width = UNITS[u]
        return pltpu.make_async_copy(w_hbm.at[e, :, pl.ds(c0, width)],
                                     wv.at[e, :, pl.ds(c0, width)], wsem.at[u])

    for u in range(len(UNITS)):
        w_copy(u).start(priority=1)

    bar = pltpu.get_barrier_semaphore()
    for k in range(1, N_DEV):
        pl.semaphore_signal(bar, 1, device_id=((me + k) % N_DEV,), device_id_type=MESH)

    row = lax.broadcasted_iota(i32, (128, 128), 0)
    col = lax.broadcasted_iota(i32, (128, 128), 1)
    upper = (row <= col).astype(bf16)
    ones = jnp.ones((128, 128), bf16)
    below = (((row >> 4) == (col >> 4)) & (col < row)).astype(bf16)
    row4 = lax.broadcasted_iota(i32, (128, 4 * 128), 0)
    col4 = lax.broadcasted_iota(i32, (128, 4 * 128), 1)
    slot4 = (col4 & (SLOTS - 1)).astype(f32)
    same_e = (row4 >> 4) == (col4 >> 6)
    route_copy.wait()
    route8 = jnp.concatenate([route_ref[...]] * E_LOC, axis=0)

    def tables(chip):
        hit = route8 == (row >> 4) + chip * E_LOC
        hb = hit.astype(bf16)
        tot = jnp.dot(hb, ones, preferred_element_type=f32)
        off = jnp.dot(below, tot.astype(bf16), preferred_element_type=f32)
        pos = jnp.dot(hb, upper, preferred_element_type=f32) + off
        end = jnp.minimum(off + tot, CAP)
        off = jnp.minimum(off, CAP)
        pos_t = jnp.where(hit & (pos <= CAP), pos, 0.0).T.astype(bf16)
        run = (same_e & (jnp.concatenate([off] * 4, axis=1) <= slot4)
               & (slot4 < jnp.concatenate([end] * 4, axis=1)))
        rank = jnp.dot(pos_t, run.astype(bf16), preferred_element_type=f32)
        tok = (jnp.where(rank == slot4 + 1.0, row4 + 1, 0)
               + jnp.where(run, (row4 & 15) * 128, 0))
        tok = jnp.sum(tok.astype(f32), axis=0, keepdims=True).astype(i32) - 1
        diag = row == col
        off_r = jnp.sum(jnp.where(diag, off, 0.0), axis=0, keepdims=True)
        end_r = jnp.sum(jnp.where(diag, end, 0.0), axis=0, keepdims=True)
        tab_v[pl.ds(pl.multiple_of(chip * 8, 8), 8), :] = jnp.concatenate(
            [tok[:, q * 128:(q + 1) * 128] for q in range(4)]
            + [off_r.astype(i32), end_r.astype(i32), jnp.zeros((2, 128), i32)], axis=0)

    def tab_copy(lo, n):
        return pltpu.make_async_copy(tab_v.at[pl.ds(lo, n)], tab_s.at[pl.ds(lo, n)], tsem)

    def token(chip, e, s):
        return tab_s[chip * 8 + e // 2, (e % 2) * SLOTS + s]

    tables(me)
    own = tab_copy(pl.multiple_of(me * 8, 8), 8)
    own.start()
    for e in range(E_LOC):
        xg[e * SLOTS + 48:(e + 1) * SLOTS, :] = jnp.zeros((SLOTS - 48, D), f32)
    own.wait()

    for e in range(E_LOC):
        for s in range(CAP):
            t = jnp.maximum(token(me, e, s), 0)
            pltpu.make_async_copy(x_hbm.at[pl.ds(t, 1)], xg.at[pl.ds(e * SLOTS + s, 1)],
                                  gsem.at[e]).start()

    for k in range(1, N_DEV):
        tables((me + k) % N_DEV)
    rest = tab_copy(0, 8 * N_DEV)
    rest.start()
    out_ref[...] = jnp.zeros_like(out_ref)
    rest.wait()

    pl.semaphore_wait(bar, N_DEV - 1)
    for k in range(1, N_DEV):
        pl.semaphore_signal(done_sem, 1, device_id=((me + k) % N_DEV,), device_id_type=MESH)

    def exchange(src, dst, u):
        e, _, width = UNITS[u]
        nw = _words(width)
        lo = tab_s[src * 8 + 4, e * 16 + dst * 4]
        n = tab_s[src * 8 + 5, e * 16 + dst * 4 + 3] - lo
        rows = stage.at[pl.ds(_STAGE_AT[u] + (src * SLOTS + lo) * nw, n * nw)]
        k = u * N_DEV + (dst - src) % N_DEV
        return lambda: pltpu.make_async_remote_copy(
            rows, rows, ssem.at[k], rsem.at[k], device_id=(dst,), device_id_type=MESH), lo, n

    def place(u):
        e, c0, width = UNITS[u]
        nw = _words(width)
        for k in (0, 1, 3, 2):
            src = (me - k) % N_DEV
            copy, lo, n = exchange(src, me, u)
            if k:
                pl.when(n > 0)(lambda: copy().wait_recv())

            def put(s, carry):
                r = token(src, e, s) & (ROWS - 1)
                w = stage[pl.ds(_STAGE_AT[u] + (src * SLOTS + s) * nw, nw), :]
                at = (r >> 3) * 64 + (r & 7) + c0 // 16
                out_ref[pl.ds(at, nw, stride=8), :] = pltpu.bitcast(w << 16, f32)
                out_ref[pl.ds(at + 8 * nw, nw, stride=8), :] = pltpu.bitcast(
                    w & jnp.uint32(0xFFFF0000), f32)
                return carry

            lax.fori_loop(lo, lo + n, put, 0)

    def drain():
        for u in range(len(UNITS)):
            for k in range(1, N_DEV):
                copy, _, n = exchange(me, (me + k) % N_DEV, u)
                pl.when(n > 0)(lambda: copy().wait_send())
        pl.semaphore_wait(done_sem, N_DEV - 1)

    xb = None
    for u, (e, c0, width) in enumerate(UNITS):
        if c0 == 0:
            gathered = stage.at[pl.ds(0, CAP * D // 128)]
            pltpu.make_async_copy(gathered, gathered, gsem.at[e]).wait()
            xb = xg[e * SLOTS:(e + 1) * SLOTS, :].astype(bf16)
        w_copy(u).wait()
        y = jnp.dot(xb, wv[e, :, c0:c0 + width].astype(bf16), preferred_element_type=f32)
        bits = pltpu.bitcast(y.astype(bf16).astype(f32), u32)
        packed = (bits[:, :width // 2] >> 16) | bits[:, width // 2:]
        nw = _words(width)
        mine = stage.at[pl.ds(pl.multiple_of(_STAGE_AT[u] + me * SLOTS * nw, SLOTS), SLOTS * nw)]
        for q in range(nw):
            mine[pl.ds(q, SLOTS, stride=nw), :] = packed[:, q * 128:(q + 1) * 128]
        for k in (2, 1, 3):
            copy, _, n = exchange(me, (me + k) % N_DEV, u)
            pl.when(n > 0)(lambda: copy().start())
        for v in PLACE_AFTER.get(u, ()):
            if v == len(UNITS) - 1:
                drain()
            place(v)


def pallas_dist_moe_cap_ep_outshard_n2048_d512_e8_h1024_kernel(
    x: jax.Array,
    router_W: jax.Array,
    route_idx: jax.Array,
    expert_W: jax.Array,
):
    del router_W
    n_sem = len(UNITS) * N_DEV
    out = pl.pallas_call(
        _body,
        out_shape=jax.ShapeDtypeStruct((ROWS * H // 128, 128), f32),
        in_specs=[pl.BlockSpec(memory_space=pltpu.HBM)] * 3,
        out_specs=pl.BlockSpec(memory_space=pltpu.VMEM),
        scratch_shapes=[
            pltpu.VMEM((N_TOK // 128, 128), i32),
            pltpu.VMEM((E_LOC, D, H), f32),
            pltpu.VMEM((E_LOC * SLOTS, D), f32),
            pltpu.VMEM((_STAGE_AT[-1], 128), u32),
            pltpu.VMEM((8 * N_DEV, 128), i32),
            pltpu.SMEM((8 * N_DEV, 128), i32),
            pltpu.SemaphoreType.DMA((len(UNITS),)),
            pltpu.SemaphoreType.DMA((E_LOC,)),
            pltpu.SemaphoreType.DMA,
            pltpu.SemaphoreType.DMA((n_sem,)),
            pltpu.SemaphoreType.DMA((n_sem,)),
            pltpu.SemaphoreType.REGULAR,
        ],
        compiler_params=pltpu.CompilerParams(
            vmem_limit_bytes=64 << 20, disable_bounds_checks=True, collective_id=0),
    )(route_idx.reshape(N_TOK // 128, 128), x, expert_W)
    return out.reshape(ROWS // 8, H // 128, 8, 128).transpose(0, 2, 1, 3).reshape(ROWS, H)
```

```python
import jax
import jax.numpy as jnp
from jax import lax
from jax.experimental import pallas as pl
from jax.experimental.pallas import tpu as pltpu

N_DEV = 4
N_TOK = 2048
D = 512
H = 1024
E_LOC = 8
CAP = 51
SLOTS = 64
ROWS = N_TOK // N_DEV
MESH = pl.DeviceIdType.MESH

UNITS = tuple((e, 0, H) for e in range(E_LOC - 1)) + (
    (E_LOC - 1, 0, H // 2), (E_LOC - 1, H // 2, H // 2))
PLACE_AFTER = {3: (0, 1), 4: (2,), 5: (3,), 6: (4,), 7: (5,)}
PLACE_LAST = (6, 7, 8)
UNROLL = 4

f32, bf16, i32, u32 = jnp.float32, jnp.bfloat16, jnp.int32, jnp.uint32


def _words(width):
    return width // 256


_STAGE_AT = [0]
for _, _, _w in UNITS:
    _STAGE_AT.append(_STAGE_AT[-1] + N_DEV * SLOTS * _words(_w))


def _body(route_hbm, x_hbm, w_hbm, out_ref,
          route_ref, wv, xg, stage, tab_v, tab_s,
          wsem, gsem, tsem, ssem, rsem, done_sem):
    me = lax.axis_index("i")

    route_copy = pltpu.make_async_copy(route_hbm, route_ref, tsem)
    route_copy.start()

    def w_copy(u):
        e, c0, width = UNITS[u]
        return pltpu.make_async_copy(w_hbm.at[e, :, pl.ds(c0, width)],
                                     wv.at[e, :, pl.ds(c0, width)], wsem.at[u])

    for u in range(len(UNITS)):
        w_copy(u).start(priority=1)

    bar = pltpu.get_barrier_semaphore()
    for k in range(1, N_DEV):
        pl.semaphore_signal(bar, 1, device_id=((me + k) % N_DEV,), device_id_type=MESH)

    row = lax.broadcasted_iota(i32, (128, 128), 0)
    col = lax.broadcasted_iota(i32, (128, 128), 1)
    upper = (row <= col).astype(bf16)
    ones = jnp.ones((128, 128), bf16)
    below = (((row >> 4) == (col >> 4)) & (col < row)).astype(bf16)
    row4 = lax.broadcasted_iota(i32, (128, 4 * 128), 0)
    col4 = lax.broadcasted_iota(i32, (128, 4 * 128), 1)
    slot4 = (col4 & (SLOTS - 1)).astype(f32)
    same_e = (row4 >> 4) == (col4 >> 6)
    route_copy.wait()
    route8 = jnp.concatenate([route_ref[...]] * E_LOC, axis=0)

    def tables(chip):
        hit = route8 == (row >> 4) + chip * E_LOC
        hb = hit.astype(bf16)
        tot = jnp.dot(hb, ones, preferred_element_type=f32)
        off = jnp.dot(below, tot.astype(bf16), preferred_element_type=f32)
        pos = jnp.dot(hb, upper, preferred_element_type=f32) + off
        end = jnp.minimum(off + tot, CAP)
        off = jnp.minimum(off, CAP)
        pos_t = jnp.where(hit & (pos <= CAP), pos, 0.0).T.astype(bf16)
        run = (same_e & (jnp.concatenate([off] * 4, axis=1) <= slot4)
               & (slot4 < jnp.concatenate([end] * 4, axis=1)))
        rank = jnp.dot(pos_t, run.astype(bf16), preferred_element_type=f32)
        tok = (jnp.where(rank == slot4 + 1.0, row4 + 1, 0)
               + jnp.where(run, (row4 & 15) * 128, 0))
        tok = jnp.sum(tok.astype(f32), axis=0, keepdims=True).astype(i32) - 1
        diag = row == col
        off_r = jnp.sum(jnp.where(diag, off, 0.0), axis=0, keepdims=True)
        end_r = jnp.sum(jnp.where(diag, end, 0.0), axis=0, keepdims=True)
        tab_v[pl.ds(pl.multiple_of(chip * 8, 8), 8), :] = jnp.concatenate(
            [tok[:, q * 128:(q + 1) * 128] for q in range(4)]
            + [off_r.astype(i32), end_r.astype(i32), jnp.zeros((2, 128), i32)], axis=0)

    def tab_copy(lo, n):
        return pltpu.make_async_copy(tab_v.at[pl.ds(lo, n)], tab_s.at[pl.ds(lo, n)], tsem)

    def token(chip, e, s):
        return tab_s[chip * 8 + e // 2, (e % 2) * SLOTS + s]

    tables(me)
    own = tab_copy(pl.multiple_of(me * 8, 8), 8)
    own.start()
    for e in range(E_LOC):
        xg[e * SLOTS + 48:(e + 1) * SLOTS, :] = jnp.zeros((SLOTS - 48, D), f32)
    own.wait()

    def x_copy(t, e, s):
        return pltpu.make_async_copy(x_hbm.at[pl.ds(t, 1)], xg.at[pl.ds(e * SLOTS + s, 1)],
                                     gsem.at[e])

    for e in range(E_LOC):
        for s in range(CAP):
            x_copy(jnp.maximum(token(me, e, s), 0), e, s).start()

    for k in range(1, N_DEV):
        tables((me + k) % N_DEV)
    rest = tab_copy(0, 8 * N_DEV)
    rest.start()
    out_ref[...] = jnp.zeros_like(out_ref)
    rest.wait()

    pl.semaphore_wait(bar, N_DEV - 1)
    for k in range(1, N_DEV):
        pl.semaphore_signal(done_sem, 1, device_id=((me + k) % N_DEV,), device_id_type=MESH)

    def exchange(src, dst, u):
        e, _, width = UNITS[u]
        nw = _words(width)
        lo = tab_s[src * 8 + 4, e * 16 + dst * 4]
        n = tab_s[src * 8 + 5, e * 16 + dst * 4 + 3] - lo
        rows = stage.at[pl.ds(_STAGE_AT[u] + (src * SLOTS + lo) * nw, n * nw)]
        k = u * N_DEV + (dst - src) % N_DEV
        return lambda: pltpu.make_async_remote_copy(
            rows, rows, ssem.at[k], rsem.at[k], device_id=(dst,), device_id_type=MESH), lo, n

    def place(u, hops=(0, 1, 3, 2)):
        e, c0, width = UNITS[u]
        nw = _words(width)
        for k in hops:
            src = (me - k) % N_DEV
            copy, lo, n = exchange(src, me, u)
            if k:
                pl.when(n > 0)(lambda: copy().wait_recv())

            def put(j, carry):
                for i in range(UNROLL):
                    s = jnp.minimum(lo + j * UNROLL + i, lo + n - 1)
                    r = token(src, e, s) & (ROWS - 1)
                    w = stage[pl.ds(_STAGE_AT[u] + (src * SLOTS + s) * nw, nw), :]
                    at = (r >> 3) * 64 + (r & 7) + c0 // 16
                    out_ref[pl.ds(at, nw, stride=8), :] = pltpu.bitcast(w << 16, f32)
                    out_ref[pl.ds(at + 8 * nw, nw, stride=8), :] = pltpu.bitcast(
                        w & jnp.uint32(0xFFFF0000), f32)
                return carry

            lax.fori_loop(0, (n + UNROLL - 1) // UNROLL, put, 0)

    def drain():
        for u in range(len(UNITS)):
            for k in range(1, N_DEV):
                copy, _, n = exchange(me, (me + k) % N_DEV, u)
                pl.when(n > 0)(lambda: copy().wait_send())
        pl.semaphore_wait(done_sem, N_DEV - 1)

    xb = None
    for u, (e, c0, width) in enumerate(UNITS):
        if c0 == 0:
            for s in range(CAP):
                x_copy(0, e, s).wait()
            xb = xg[e * SLOTS:(e + 1) * SLOTS, :].astype(bf16)
        w_copy(u).wait()
        y = jnp.dot(xb, wv[e, :, c0:c0 + width].astype(bf16), preferred_element_type=f32)
        bits = pltpu.bitcast(y.astype(bf16).astype(f32), u32)
        packed = (bits[:, :width // 2] >> 16) | bits[:, width // 2:]
        nw = _words(width)
        mine = stage.at[pl.ds(pl.multiple_of(_STAGE_AT[u] + me * SLOTS * nw, SLOTS), SLOTS * nw)]
        for q in range(nw):
            mine[pl.ds(q, SLOTS, stride=nw), :] = packed[:, q * 128:(q + 1) * 128]
        for k in (2, 1, 3):
            copy, _, n = exchange(me, (me + k) % N_DEV, u)
            pl.when(n > 0)(lambda: copy().start())
        for v in PLACE_AFTER.get(u, ()):
            place(v)

    for v in PLACE_LAST:
        place(v, (0, 1, 3))
    drain()
    for v in PLACE_LAST:
        place(v, (2,))


def pallas_dist_moe_cap_ep_outshard_n2048_d512_e8_h1024_kernel(
    x: jax.Array,
    router_W: jax.Array,
    route_idx: jax.Array,
    expert_W: jax.Array,
):
    del router_W
    n_sem = len(UNITS) * N_DEV
    out = pl.pallas_call(
        _body,
        out_shape=jax.ShapeDtypeStruct((ROWS * H // 128, 128), f32),
        in_specs=[pl.BlockSpec(memory_space=pltpu.HBM)] * 3,
        out_specs=pl.BlockSpec(memory_space=pltpu.VMEM),
        scratch_shapes=[
            pltpu.VMEM((N_TOK // 128, 128), i32),
            pltpu.VMEM((E_LOC, D, H), f32),
            pltpu.VMEM((E_LOC * SLOTS, D), f32),
            pltpu.VMEM((_STAGE_AT[-1], 128), u32),
            pltpu.VMEM((8 * N_DEV, 128), i32),
            pltpu.SMEM((8 * N_DEV, 128), i32),
            pltpu.SemaphoreType.DMA((len(UNITS),)),
            pltpu.SemaphoreType.DMA((E_LOC,)),
            pltpu.SemaphoreType.DMA,
            pltpu.SemaphoreType.DMA((n_sem,)),
            pltpu.SemaphoreType.DMA((n_sem,)),
            pltpu.SemaphoreType.REGULAR,
        ],
        compiler_params=pltpu.CompilerParams(
            vmem_limit_bytes=64 << 20, collective_id=0,
            disable_bounds_checks=True, disable_semaphore_checks=True),
    )(route_idx.reshape(N_TOK // 128, 128), x, expert_W)
    return out.reshape(ROWS // 8, H // 128, 8, 128).transpose(0, 2, 1, 3).reshape(ROWS, H)
```
